```python
import numpy as np

kernel_name = "dist_mlp2_tp_i_m512_h1024_out512"

def setup_inputs():
    x = np.random.randn(512, 512).astype(np.float32)
    W1 = np.random.randn(512, 4096).astype(np.float32)
    W2 = np.random.randn(4096, 512).astype(np.float32)
    return {"x": x, "W1": W1, "W2": W2}

def reference(x: np.ndarray, W1: np.ndarray, W2: np.ndarray) -> np.ndarray:
    h = x @ W1
    h = np.maximum(h, 0.0)
    return h @ W2
```

```python
import contextlib
import jax
import jax.numpy as jnp
from jax import lax
from jax.experimental import pallas as pl
from jax.experimental.pallas import tpu as pltpu

M, K, H, N = 512, 512, 1024, 512
RB = 128
CB = 128
NC = N // CB
BF = jnp.bfloat16
F32 = jnp.float32


def make(scoped=False, R0=64, KB=128):
    scope = jax.named_scope if scoped else (lambda n: contextlib.nullcontext())
    NK = K // KB
    R1 = RB - R0
    E = 2 * RB + 2 * R0

    def body(x_hbm, w1_hbm, w2_hbm, out,
             xv, w1v, w2v, w1b, w2b, acc, hb, s1, r1, s2, r2, pk,
             ld_sem, send_sem, recv_sem):
        me = lax.axis_index("i")
        nbr = (me ^ 1, me ^ 3)
        a = (me ^ (me >> 1)) & 1
        b = me >> 1
        rows = ((1 - a) * RB, (3 - b) * RB, a * RB, (2 + b) * RB)
        rows = [pl.multiple_of(r, RB) for r in rows]
        nsem = [0]
        def ld(src, dst):
            c = pltpu.make_async_copy(src, dst, ld_sem.at[nsem[0]]); nsem[0] += 1
            c.start()
            return c
        xe = [ld(x_hbm.at[pl.ds(rows[j], RB)], xv.at[pl.ds(j * RB, RB)]) for j in range(2)]
        if R0:
            xe += [ld(x_hbm.at[pl.ds(rows[2 + j], R0)], xv.at[pl.ds(2 * RB + j * R0, R0)]) for j in range(2)]
        w1c = [ld(w1_hbm.at[pl.ds(j * KB, KB)], w1v.at[pl.ds(j * KB, KB)]) for j in range(NK)]
        w2c = [[ld(w2_hbm.at[pl.ds(h * 512, 512), pl.ds(j * CB, CB)], w2v.at[j, pl.ds(h * 512, 512)]) for h in range(2)] for j in range(NC)]
        if R1:
            xl = [ld(x_hbm.at[pl.ds(pl.multiple_of(rows[2 + j] + R0, 16), R1)], xv.at[pl.ds(E + j * R1, R1)]) for j in range(2)]

        bar = pltpu.get_barrier_semaphore()
        for d in nbr:
            pl.semaphore_signal(bar, 1, device_id=(d,), device_id_type=pl.DeviceIdType.MESH)

        nr = [0]
        started = []
        def rdma(src, dst, d):
            k = nr[0]; nr[0] += 1
            c = pltpu.make_async_remote_copy(src, dst, send_sem.at[k], recv_sem.at[k],
                                             device_id=(d,), device_id_type=pl.DeviceIdType.MESH)
            c.start(); started.append(c)
            return c

        with scope("wait_xe"):
            for c in xe: c.wait()
        for j in range(NK):
            with scope(f"wait_w1_{j}"):
                w1c[j].wait()
            w = w1v[j * KB:(j + 1) * KB, :].astype(BF)
            w1b[j * KB:(j + 1) * KB, :] = w
            h = jnp.dot(xv[0:E, j * KB:(j + 1) * KB].astype(BF), w, preferred_element_type=F32)
            if j > 0:
                h = h + acc[...]
            if j < NK - 1:
                acc[...] = h
            else:
                hb[0:E, :] = jnp.maximum(h, 0.0).astype(BF)
        c1 = {}; c2 = {}; c3 = []
        def stage2(c, part, p):
            r, n = (0, R0) if part == 0 else (R0, R1)
            for l in range(2):
                if part == 0 or not R0:
                    with scope(f"wait_r1_{c}_{l}"):
                        c1[c, l].wait_recv()
                s2[c, l, r:r + n] = (p[l * n:(l + 1) * n] + r1[c, l, r:r + n].astype(F32)).astype(BF)
                c2[c, l, part] = rdma(s2.at[c, l, pl.ds(r, n)], r2.at[c, l, pl.ds(r, n)], nbr[1 - l])
        def stage3(c, part):
            r, n = (0, R0) if part == 0 else (R0, R1)
            for l in range(2):
                with scope(f"wait_r2_{c}_{l}_{part}"):
                    c2[c, l, part].wait_recv()
                dst = out.at[pl.ds(pl.multiple_of(rows[2 + l] + r, 16), n), pl.ds(c * CB, CB)]
                dst[...] = (s2[c, l, r:r + n].astype(F32) + r2[c, l, r:r + n].astype(F32)).astype(BF)
                c3.append(rdma(dst, dst, nbr[l]))
        for c in range(NC):
            p = None
            for hf in range(2):
                with scope(f"wait_w2_{c}_{hf}"):
                    w2c[c][hf].wait()
                w = w2v[c, hf * 512:(hf + 1) * 512].astype(BF)
                w2b[c, hf * 512:(hf + 1) * 512] = w
                q = jnp.dot(hb[0:E, hf * 512:(hf + 1) * 512], w, preferred_element_type=F32)
                p = q if p is None else p + q
            s1[c, 0] = p[0:RB].astype(BF)
            s1[c, 1] = p[RB:2 * RB].astype(BF)
            if R0:
                pk[c] = p[2 * RB:E]
            if c == 0:
                with scope("barrier"):
                    pl.semaphore_wait(bar, 2)
            for l in range(2):
                c1[c, l] = rdma(s1.at[c, l], r1.at[c, l], nbr[l])
        if R1:
            with scope("wait_xl"):
                for c in xl: c.wait()
            h = jnp.dot(xv[E:, :].astype(BF), w1b[...], preferred_element_type=F32)
            hb[E:, :] = jnp.maximum(h, 0.0).astype(BF)
        for c in range(NC):
            if R0:
                stage2(c, 0, pk[c])
            if R1:
                stage2(c, 1, jnp.dot(hb[E:, :], w2b[c], preferred_element_type=F32))
        for c in range(NC):
            if R0: stage3(c, 0)
            if R1: stage3(c, 1)
        with scope("wait_send"):
            for c in started: c.wait_send()
        with scope("wait_r3"):
            for c in c3: c.wait_recv()

    def fn(x, W1, W2):
        tile = pltpu.VMEM((NC, 2, RB, CB), BF)
        return pl.pallas_call(
            body,
            out_shape=jax.ShapeDtypeStruct((M, N), BF),
            in_specs=[pl.BlockSpec(memory_space=pltpu.HBM)] * 3,
            out_specs=pl.BlockSpec(memory_space=pltpu.VMEM),
            scratch_shapes=[
                pltpu.VMEM((M, K), F32), pltpu.VMEM((K, H), F32), pltpu.VMEM((NC, H, CB), F32),
                pltpu.VMEM((K, H), BF), pltpu.VMEM((NC, H, CB), BF), pltpu.VMEM((E, H), F32), pltpu.VMEM((M, H), BF),
                tile, tile, tile, tile, pltpu.VMEM((NC, max(2 * R0, 8), CB), F32),
                pltpu.SemaphoreType.DMA((32,)),
                pltpu.SemaphoreType.DMA((10 * NC,)), pltpu.SemaphoreType.DMA((10 * NC,)),
            ],
            compiler_params=pltpu.CompilerParams(collective_id=0, vmem_limit_bytes=64 << 20,
                                                 disable_semaphore_checks=True, disable_bounds_checks=True),
        )(*[pltpu.with_memory_space_constraint(a, pltpu.HBM) for a in (x, W1, W2)])
    return fn


def pallas_dist_mlp2_tp_i_m512_h1024_out512_kernel(x, W1, W2):
    return make()(x, W1, W2)
```

```python
import functools

import jax
import jax.numpy as jnp
from jax import lax
from jax.experimental import pallas as pl
from jax.experimental.pallas import tpu as pltpu

M, K, H, N = 512, 512, 1024, 512
G = 16
L = 128
HALF = M // G // 2
BF16, F32 = jnp.bfloat16, jnp.float32

WALK, WALK_ROWS = 64, 16
MXU_LAG = 176

FIRST, MID, LAST = 0, 1, 2
MIRROR = 3


def up(*spans, k=(0, K // L), n=(0, H // L)):
    return "up", spans, k, n


def down(c, *spans, k=(0, H // L)):
    return "down", spans, k, c


def send(*counts):
    return "send", counts


FENCE = ("fence",)

ROOT_FIRST = (8, 8, 6, 0)
STREAM = (
    (0, 0, 8), (1, 5, 8), (1, 0, 5), (0, 8, 10), (1, 8, 10), (2, 4, 6), (1, 10, 12), (0, 10, 12),
    (2, 0, 3), (2, 6, 12), (2, 3, 4), (1, 13, 15), (0, 13, 15), (3, 0, 16), (0, 15, 16),
    (1, 12, 13), (1, 15, 16), (2, 12, 16), (0, 12, 13),
)
RELAYED_BY_FIRST = 14
X_ROWS = {
    (FIRST, MID): ((29, 30), (25, 29), (30, 32)),
    (MID, FIRST): ((19, 21), (17, 19), (16, 17)),
    (MID, LAST): ((19, 28),),
    (LAST, MID): ((0, 1), (17, 19), (16, 17), (1, 8)),
}
OWN_TILES = {
    (FIRST, MID): (
        (0, 8, 12), (0, 12, 16), (1, 8, 16), (2, 6, 12), (2, 12, 16), (3, 6, 15), (3, 15, 16),
        (3, 0, 2), (3, 2, 6),
    ),
    (MID, FIRST): (
        (0, 22, 24), (0, 18, 22), (0, 16, 18), (1, 17, 18), (1, 18, 19), (1, 16, 17), (1, 20, 23),
        (1, 23, 24), (1, 19, 20), (2, 20, 22), (2, 16, 19), (2, 19, 20),
    ),
    (MID, LAST): (
        (0, 24, 25), (0, 25, 28), (0, 28, 30), (1, 24, 25), (1, 25, 27), (1, 27, 28), (1, 28, 31),
        (1, 31, 32), (0, 30, 32), (2, 26, 27), (2, 22, 23), (2, 23, 26), (2, 27, 31), (2, 31, 32),
        (3, 16, 19), (3, 19, 23), (3, 23, 27), (3, 27, 31), (3, 31, 32),
    ),
}
W1_BLOCKS = tuple(("w1", k, k + 1) for k in range(K // L))
LOADS = {
    FIRST: (
        ("x", 5, 16), *W1_BLOCKS, (0, 0, 8), (1, 0, 8), (2, 0, 8), (3, 0, 8),
    ),
    MID: (
        ("x", 19, 25), *W1_BLOCKS, (0, 0, 8), (1, 0, 4), (1, 4, 8), (2, 0, 4), (2, 4, 8),
        (3, 0, 8), ("x", 8, 16),
    ),
    LAST: (
        ("x", 0, 1), ("x", 2, 3), ("x", 1, 2), *W1_BLOCKS, (0, 0, 8), (1, 0, 4), (1, 4, 8),
        (2, 0, 8), (3, 0, 8), ("x", 12, 16),
    ),
}
PROGRAM = {
    FIRST: (
        send(7), up((5, 16), k=(0, 2)), FENCE,
        up((5, 16), k=(2, 3)), FENCE,
        up((5, 16), k=(3, 4)), FENCE,
        down(0, (8, 12)), down(0, (12, 16)), send(1), FENCE,
        send(1), down(1, (8, 16)), FENCE,
        send(1), down(2, (6, 12)), down(2, (12, 16)), send(1), up((0, 2)), send(1),
        down(3, (6, 15)), FENCE,
        send(1), up((2, 5)), down(3, (0, 2), (15, 16)), down(3, (2, 6)), send(2), FENCE,
        send(1), down(0, (0, 8)), FENCE,
        send(6), down(2, (0, 6)), FENCE,
        send(8), down(1, (0, 8)), FENCE,
    ),
    MID: (
        send(2, 6), send(0, 1), up((0, 1), (19, 26), (29, 30), k=(0, 2)), FENCE,
        send(1, 1), send(0, 1), up((17, 18), (26, 28), k=(0, 2)),
        up((0, 1), (17, 18), (19, 28), (29, 30), k=(2, 3)), FENCE,
        send(2, 0), up((16, 17), (18, 19), (28, 29), k=(0, 3)), up((0, 1), (16, 30), k=(3, 4)),
        FENCE,
        down(0, (22, 25)), down(0, (25, 28)), down(0, (18, 22)), send(1, 1),
        up((1, 2), (30, 32), k=(0, 1)), send(0, 1), down(0, (16, 18), (28, 30)), send(1, 0),
        down(1, (17, 18), (22, 23), (24, 25), k=(0, 4)), up((1, 2), (30, 32), k=(1, 4)),
        send(1, 1), down(1, (17, 18), (22, 23), (24, 25), k=(4, 8)), down(1, (18, 19), (25, 27)),
        down(1, (16, 17), (20, 22), (27, 28)), send(1, 1), down(1, (28, 31)), send(1, 1),
        down(1, (0, 1), (19, 20), (23, 24), (31, 32)), send(2, 1), down(0, (0, 1), (30, 32)),
        send(0, 1), down(2, (20, 22), (26, 27), k=(0, 4)), up((2, 5)), send(2, 2),
        down(2, (20, 22), (26, 27), k=(4, 8)), down(2, (16, 19), (22, 23)), down(2, (23, 26)),
        send(1, 1), down(2, (19, 20), (27, 32)), send(1, 1), up((5, 8), n=(0, 2)), send(0, 1),
        down(0, (1, 5)), send(1, 2), up((5, 8), n=(2, 8)), send(1, 0), down(1, (1, 5)), send(2, 0),
        down(3, (16, 19)), send(1, 0), down(0, (5, 8)), send(1, 0), down(3, (19, 27)), send(1, 1),
        down(1, (5, 8)), send(2, 0), up((8, 13), n=(6, 8)), send(0, 2), up((8, 13), n=(4, 6)),
        send(2, 0), up((8, 13), k=(0, 2), n=(0, 4)), send(1, 0), up((8, 13), k=(2, 4), n=(0, 4)),
        send(1, 0), down(3, (27, 32)), send(2, 0), down(1, (8, 12)), send(1, 0), down(0, (8, 12)),
        send(1, 2), down(2, (0, 6)), send(1, 0), down(3, (0, 5), k=(0, 4)), send(2, 1),
        up((13, 16), n=(2, 8)), send(1, 1), up((13, 16), n=(0, 2)), send(2, 2), down(2, (6, 13)),
        send(1, 0), down(3, (11, 16), k=(0, 4)), send(1, 1), down(3, (5, 11), k=(0, 4)),
        send(1, 1), down(2, (13, 16)), send(1, 0), down(0, (12, 16)), send(1, 1),
        down(1, (12, 16)), send(0, 1), down(3, (0, 5), k=(4, 8)), send(2, 0), FENCE,
        send(2, 2), down(3, (5, 16), k=(4, 8)), send(1, 1), FENCE,
    ),
    LAST: (
        send(1), send(5), send(1), send(1), up((0, 5), k=(0, 1)), FENCE,
        send(1), up((5, 6), k=(0, 1)), up((0, 6), k=(1, 3)), FENCE,
        send(1), send(1), up((6, 8), k=(0, 3)), up((0, 8), k=(3, 4)), FENCE,
        down(0, (0, 2)), down(0, (2, 5)), send(2), down(0, (5, 8)), send(3), up((8, 10), n=(0, 4)),
        send(3), down(1, (5, 8), k=(0, 4)), FENCE,
        down(1, (5, 8), k=(4, 8)), down(1, (3, 5)), down(1, (0, 3), k=(0, 4)), send(3),
        down(1, (0, 3), k=(4, 8)), up((8, 10), n=(4, 8)), send(5),
        up((10, 12), k=(0, 2), n=(0, 6)), down(0, (8, 10)), down(1, (8, 10)),
        up((10, 12), n=(6, 8)), send(2), up((10, 12), k=(2, 4), n=(0, 6)), send(1),
        down(2, (4, 6)), send(1), down(1, (10, 12)), send(1), down(0, (10, 12)), send(1),
        down(2, (0, 2)), send(2), down(2, (2, 4)), send(2), down(2, (6, 12)), send(3),
        up((13, 15), k=(0, 2)), send(1), up((13, 15), k=(2, 4), n=(0, 4)), send(2),
        up((13, 15), k=(2, 4), n=(4, 8)), send(2), down(3, (0, 10), k=(0, 4)), send(2),
        down(1, (13, 15)), down(0, (13, 15)), down(3, (0, 3), k=(4, 8)), send(2),
        down(3, (3, 10), k=(4, 8)), send(2), FENCE,
        send(5), up((12, 13), (15, 16)), FENCE,
        send(5), down(3, (10, 16)), FENCE,
        send(4), down(1, (12, 13), (15, 16)), send(1), down(0, (12, 13), (15, 16)), FENCE,
        send(4), down(2, (12, 16)), FENCE,
    ),
}


def _queues():
    stream = [(c, g, g + 1) for c, g0, g1 in STREAM for g in range(g0, g1)]
    at_first = [t for t in stream if t[1] < ROOT_FIRST[t[0]]]
    at_mid = [t for t in stream if t not in at_first]
    other = lambda t: (t[0], t[1] + HALF, t[2] + HALF)
    q = {
        link: [("x", None, g, g + 1) for g0, g1 in X_ROWS[link] for g in range(g0, g1)]
        + [("own", *t) for t in OWN_TILES.get(link, ())]
        for link in X_ROWS
    }
    q[LAST, MID] += [("own" if t in at_first else "sum", *t) for t in stream]
    q[MID, FIRST] += [("sum" if t in at_first else "total", *t) for t in stream]
    q[FIRST, MID] += [("total", *u) for t in at_first for u in (t, other(t))]
    q[FIRST, MID] += [("relay", *other(t)) for t in at_mid[:RELAYED_BY_FIRST]]
    q[LAST, MID] += [("relay", *other(t)) for t in at_mid[RELAYED_BY_FIRST:]]
    q[MID, LAST] += [("total", *t) for t in at_mid] + [("relay", *t) for t in at_first]
    return q


def _rows(g0, g1):
    return pl.ds(g0 * G, (g1 - g0) * G)


def _swap(g0, g1):
    return g0 ^ HALF, (g0 ^ HALF) + g1 - g0


def _run(role, mirrored, barrier,
         x_hbm, w1_hbm, w2_hbm, out,
         x32, x16, w1_32, w1_16, w2_32, pre, h16, part, outbox, inbox,
         load_sems, send_sems, recv_sems, fence_sem):
    queues = _queues()
    peers = (FIRST, LAST) if role == MID else (MID, MIRROR)
    links = [link for link in queues if link[0] == role]

    if role == MID:
        base = [pl.multiple_of(b * (M // 2), M // 2) for b in (mirrored, 1 - mirrored)]
        global_rows = lambda g0, g1: pl.ds(base[g0 // HALF] + g0 % HALF * G, (g1 - g0) * G)
        halves = list
    else:
        global_rows = _rows
        halves = lambda spans: [*spans, *(_swap(*s) for s in spans)]

    def queue(src, dst):
        return queues[MID if src == MIRROR else src, MID if dst == MIRROR else dst]

    def message(src, dst, i):
        kind, c, *span = queue(src, dst)[i]
        return kind, c, *(_swap(*span) if MIRROR in (src, dst) else span)

    def remote_copy(src, dst, i):
        kind, c, g0, g1 = message(src, dst, i)
        side = mirrored if src == role == MID else src // 2
        if src != role:
            there = _rows(g0, g1)
        else:
            there = _rows(*_swap(g0, g1)) if dst == MIRROR else global_rows(g0, g1)
        if kind == "x":
            a, b = x16.at[_rows(g0, g1)], x16.at[there]
        elif kind in ("own", "sum"):
            a, b = outbox.at[c, _rows(g0, g1)], inbox.at[side, c, there]
        else:
            a = b = out.at[global_rows(g0, g1), pl.ds(c * L, L)]
        return pltpu.make_async_remote_copy(
            a, b, send_sems.at[2 * i + dst // 2], recv_sems.at[2 * i + side],
            device_id=(dst if src == role else src,), device_id_type=pl.DeviceIdType.MESH)

    source = {}
    for src in peers:
        for i in range(len(queue(src, role))):
            kind, c, g0, g1 = message(src, role, i)
            what = {"x": "x", "own": src, "sum": src}.get(kind, "total")
            source.update({(what, c, g): (src, i) for g in range(g0, g1)})
    sent_as_is = {
        (c, g) for link in links for kind, c, *span in queues[link] if kind == "own"
        for s in halves([span]) for g in range(*s)
    }

    loads = {}
    for key in LOADS[role]:
        what, i, j = key
        sem = load_sems.at[len(loads)]
        if what == "x":
            loads[key] = [
                pltpu.make_async_copy(x_hbm.at[global_rows(*s)], x32.at[_rows(*s)], sem)
                for s in halves([(i, j)])
            ]
        elif what == "w1":
            s = pl.ds(i * L, (j - i) * L)
            loads[key] = [pltpu.make_async_copy(w1_hbm.at[s], w1_32.at[s], sem)]
        else:
            s = pl.ds(i * L // WALK, (j - i) * L // WALK)
            loads[key] = [
                pltpu.make_async_copy(w2_hbm.at[s, pl.ds(r, WALK_ROWS), pl.ds(what * L, L)],
                                      w2_32.at[what, s, pl.ds(r, WALK_ROWS)], sem)
                for r in range(0, WALK, WALK_ROWS)
            ]
        for copy in loads[key]:
            copy.start()
        if len(loads) == 1:
            for peer in peers:
                pl.semaphore_signal(barrier, 1, device_id=(peer,),
                                    device_id_type=pl.DeviceIdType.MESH)

    done = set()

    def first_time(*event):
        new = event not in done
        done.add(event)
        return new

    def wait_loads(what, i, j):
        for key in LOADS[role]:
            if key[0] == what and key[1] < j and key[2] > i and first_time("load", key):
                for copy in loads[key]:
                    copy.wait()
                if what == "x":
                    for s in halves([key[1:]]):
                        x16[_rows(*s)] = x32[_rows(*s)].astype(BF16)

    def wait_message(src, i):
        if first_time("message", src, i):
            remote_copy(src, role, i).wait_recv()

    def wait_x(g):
        if ("x", None, g) in source:
            wait_message(*source["x", None, g])
        else:
            g = g if role == MID else g % HALF
            wait_loads("x", g, g + 1)

    def w1_block(k, n):
        depth = pl.ds(k[0] * L, (k[1] - k[0]) * L)
        if not any([first_time("w1", i, n) for i in range(*k)]):
            return w1_16[n, depth]
        w = w1_32[depth, pl.ds(n * L, L)].astype(BF16)
        w1_16[n, depth] = w
        return w

    def store_up(spans, k, n, value):
        row = 0
        for g0, g1 in spans:
            at = _rows(g0, g1), pl.ds(n * L, L)
            v = value[row:row + (g1 - g0) * G]
            row += (g1 - g0) * G
            if k[0] > 0:
                v = v + pre[at]
            if k[1] < K // L:
                pre[at] = v
            else:
                h16[at] = jnp.maximum(v, 0.0).astype(BF16)

    def store_down(c, g, k, v):
        if k[0] > 0:
            v = v + part[c, _rows(g, g + 1)]
        if k[1] == H // L and (c, g) in sent_as_is:
            outbox[c, _rows(g, g + 1)] = v.astype(BF16)
        else:
            part[c, _rows(g, g + 1)] = v

    in_flight = []
    clock = 0

    def retire(needed):
        due = [i + 1 for i, (t, makes, _) in enumerate(in_flight)
               if needed is None or t <= clock - MXU_LAG or makes & needed]
        for _ in range(max(due, default=0)):
            in_flight.pop(0)[2]()

    started = {}
    position = dict.fromkeys(links, 0)

    def start(counts):
        batch = []
        for link, count in zip(links, counts):
            targets = link[1:] if role == MID else peers
            batch += [(dst, position[link] + i) for i in range(count) for dst in targets]
            position[link] += count
        batch = [(dst, i, *message(role, dst, i)) for dst, i in batch]
        retire({(c, g) for _, _, _, c, g0, g1 in batch for g in range(g0, g1)})
        later = []
        for dst, i, kind, c, g0, g1 in batch:
            if kind == "x":
                wait_x(g0)
            if first_time("barrier"):
                pl.semaphore_wait(barrier, 2)
            copy = started[dst, i] = remote_copy(role, dst, i)
            if kind in ("x", "own") and all(m[0] != dst for m in later):
                copy.start()
            else:
                later.append((dst, kind, c, g0, copy))
        for dst, kind, c, g, _ in later:
            needs = {"sum": [dst ^ 2], "total": peers, "relay": ["total"]}.get(kind, [])
            for what in needs:
                wait_message(*source[what, c, g])
        for dst, kind, c, g, _ in later:
            at = c, _rows(g, g + 1)
            if kind == "sum":
                outbox[at] = (part[at] + inbox[((dst ^ 2) // 2, *at)].astype(F32)).astype(BF16)
            elif kind == "total" and first_time("total", c, g):
                v = part[at] + inbox[(0, *at)].astype(F32) + inbox[(1, *at)].astype(F32)
                out[global_rows(g, g + 1), pl.ds(c * L, L)] = v.astype(BF16)
        for *_, copy in later:
            copy.start()

    for op, *args in PROGRAM[role]:
        if op == "send":
            start(*args)
        elif op == "fence":
            retire(None)
            pl.semaphore_signal(fence_sem, 1)
            pl.semaphore_wait(fence_sem, 1)
        else:
            spans, k, n = args
            spans = halves(spans)
            gs = [g for s in spans for g in range(*s)]
            depth = pl.ds(k[0] * L, (k[1] - k[0]) * L)
            if op == "up":
                for g in gs:
                    wait_x(g)
                wait_loads("w1", *k)
                retire(set())
                rhs = jnp.concatenate([w1_block(k, j) for j in range(*n)], axis=1)
                lhs = jnp.concatenate([x16[_rows(*s), depth] for s in spans])
                y = jnp.dot(lhs, rhs, preferred_element_type=F32)
                for j in range(n[1] - n[0]):
                    passes = pl.cdiv((k[1] - k[0]) * (j + 1), 4)
                    store = functools.partial(store_up, spans, k, n[0] + j, y[:, j * L:j * L + L])
                    in_flight.append((clock + passes * G * len(gs), {("h", g) for g in gs}, store))
            else:
                wait_loads(n, *k)
                retire({("h", g) for g in gs})
                rhs = w2_32[n, pl.ds(k[0] * L // WALK, (k[1] - k[0]) * L // WALK)]
                rhs = rhs.reshape((k[1] - k[0]) * L, L).astype(BF16)
                lhs = jnp.concatenate([h16[_rows(*s), depth] for s in spans])
                y = jnp.dot(lhs, rhs, preferred_element_type=F32)
                last_pass = clock + ((k[1] - k[0]) // 4 - 1) * G * len(gs)
                for r, g in enumerate(gs):
                    store = functools.partial(store_down, n, g, k, y[r * G:(r + 1) * G])
                    in_flight.append((last_pass + (r + 1) * G, {(n, g)}, store))
            clock = in_flight[-1][0]

    for i, link in enumerate(links):
        while position[link] < len(queues[link]):
            start([int(j == i) for j in range(len(links))])
            while role == MID and i == 0 and queues[links[1]][position[links[1]]][:3] in done:
                start([0, 1])

    for left in reversed(range(1, max(map(len, queues.values())) + 3)):
        for peer in peers:
            if 0 < left - 2 <= len(queue(role, peer)):
                started[peer, len(queue(role, peer)) - (left - 2)].wait_send()
            if left <= len(queue(peer, role)):
                wait_message(peer, len(queue(peer, role)) - left)


def _kernel(*refs):
    me = lax.axis_index("i")
    args = pltpu.get_barrier_semaphore(), *refs
    pl.when((me & 1) == 1)(lambda: _run(MID, me >> 1, *args))
    pl.when(me == LAST)(lambda: _run(LAST, None, *args))
    pl.when(me == FIRST)(lambda: _run(FIRST, None, *args))


def pallas_dist_mlp2_tp_i_m512_h1024_out512_kernel(
    x: jax.Array,
    W1: jax.Array,
    W2: jax.Array,
):
    assert (x.shape, W1.shape, W2.shape) == ((M, K), (K, H), (H, N))
    messages = 2 * max(map(len, _queues().values()))
    flags = {"XLA_TPU_RESCHEDULE_DMA_DONES": True} if jax.__version_info__ >= (0, 12) else None
    return pl.pallas_call(
        _kernel,
        out_shape=jax.ShapeDtypeStruct((M, N), BF16),
        in_specs=[pl.BlockSpec(memory_space=pltpu.HBM)] * 3,
        out_specs=pl.BlockSpec(memory_space=pltpu.VMEM),
        scratch_shapes=[
            pltpu.VMEM((M, K), F32),
            pltpu.VMEM((M, K), BF16),
            pltpu.VMEM((K, H), F32),
            pltpu.VMEM((H // L, K, L), BF16),
            pltpu.VMEM((N // L, H // WALK, WALK, L), F32),
            pltpu.VMEM((M, H), F32),
            pltpu.VMEM((M, H), BF16),
            pltpu.VMEM((N // L, M, L), F32),
            pltpu.VMEM((N // L, M, L), BF16),
            pltpu.VMEM((2, N // L, M, L), BF16),
            pltpu.SemaphoreType.DMA((max(map(len, LOADS.values())),)),
            pltpu.SemaphoreType.DMA((messages,)),
            pltpu.SemaphoreType.DMA((messages,)),
            pltpu.SemaphoreType.REGULAR,
        ],
        compiler_params=pltpu.CompilerParams(
            collective_id=0,
            vmem_limit_bytes=64 * 1024 * 1024,
            flags=flags,
            disable_bounds_checks=True,
            disable_semaphore_checks=True,
        ),
    )(x, W1, W2.reshape(H // WALK, WALK, N))
```
